```python
import numpy as np

kernel_name = "dist_rsx_agy_m2048_n1024"

def setup_inputs():
    return {"x": np.random.randn(2, 2048, 2048).astype(np.float32)}

def reference(x: np.ndarray) -> np.ndarray:
    return x.sum(axis=0)
```

```python
import jax
import jax.numpy as jnp
from jax import lax
from jax.experimental import pallas as pl
from jax.experimental.pallas import tpu as pltpu

ROWS = 64


def pallas_dist_rsx_agy_m2048_n1024_kernel(
x: jax.Array,
):
    _, m, n = x.shape
    nchunks = m // ROWS

    def body(x_hbm, out_hbm, xin, send_x, recv_x, send_y, recv_y, own_f32, oth_f32,
             ld_sems, sx_sems, rx_sems, sy_sems, ry_sems, st_sems, so_sems):
        my_x = lax.axis_index("x")
        my_y = lax.axis_index("y")
        x_nbr = (1 - my_x, my_y)
        y_nbr = (my_x, 1 - my_y)
        own_col = pl.multiple_of(my_y * n, n)
        oth_col = pl.multiple_of((1 - my_y) * n, n)

        def rows(i):
            return pl.ds(i * ROWS, ROWS)

        loads = [
            pltpu.make_async_copy(x_hbm.at[0, rows(i)], xin.at[rows(i)], ld_sems.at[i])
            for i in range(nchunks)
        ]
        xcopies = [
            pltpu.make_async_remote_copy(
                send_x.at[rows(i)], recv_x.at[rows(i)], sx_sems.at[i], rx_sems.at[i],
                device_id=x_nbr, device_id_type=pl.DeviceIdType.MESH)
            for i in range(nchunks)
        ]
        ycopies = [
            pltpu.make_async_remote_copy(
                send_y.at[rows(i)], recv_y.at[rows(i)], sy_sems.at[i], ry_sems.at[i],
                device_id=y_nbr, device_id_type=pl.DeviceIdType.MESH)
            for i in range(nchunks)
        ]
        own_st = [
            pltpu.make_async_copy(
                own_f32.at[rows(i)], out_hbm.at[rows(i), pl.ds(own_col, n)], st_sems.at[i])
            for i in range(nchunks)
        ]
        oth_st = [
            pltpu.make_async_copy(
                oth_f32.at[rows(i)], out_hbm.at[rows(i), pl.ds(oth_col, n)], so_sems.at[i])
            for i in range(nchunks)
        ]

        for c in loads:
            c.start()

        def stage_x(i):
            loads[i].wait()
            send_x[rows(i), :] = xin[rows(i), :].astype(jnp.bfloat16)
            xcopies[i].start()

        def stage_y(i):
            xcopies[i].wait_recv()
            s = xin[rows(i), :] + recv_x[rows(i), :].astype(jnp.float32)
            send_y[rows(i), :] = s.astype(jnp.bfloat16)
            ycopies[i].start()
            own_f32[rows(i), :] = s
            own_st[i].start()

        def stage_o(i):
            ycopies[i].wait_recv()
            oth_f32[rows(i), :] = recv_y[rows(i), :].astype(jnp.float32)
            oth_st[i].start()

        AHEAD = 3
        LAG = 2
        for t in range(-AHEAD, nchunks + LAG):
            if 0 <= t + AHEAD < nchunks:
                stage_x(t + AHEAD)
            if 0 <= t < nchunks:
                stage_y(t)
            if 0 <= t - LAG < nchunks:
                stage_o(t - LAG)

        for i in range(nchunks):
            xcopies[i].wait_send()
            ycopies[i].wait_send()
            own_st[i].wait()
            oth_st[i].wait()

    return pl.pallas_call(
        body,
        out_shape=jax.ShapeDtypeStruct((m, 2 * n), jnp.float32),
        in_specs=[pl.BlockSpec(memory_space=pl.ANY)],
        out_specs=pl.BlockSpec(memory_space=pl.ANY),
        scratch_shapes=[
            pltpu.VMEM((m, n), jnp.float32),
            pltpu.VMEM((m, n), jnp.bfloat16),
            pltpu.VMEM((m, n), jnp.bfloat16),
            pltpu.VMEM((m, n), jnp.bfloat16),
            pltpu.VMEM((m, n), jnp.bfloat16),
            pltpu.VMEM((m, n), jnp.float32),
            pltpu.VMEM((m, n), jnp.float32),
        ] + [pltpu.SemaphoreType.DMA((nchunks,))] * 7,
        compiler_params=pltpu.CompilerParams(vmem_limit_bytes=64 * 1024 * 1024),
    )(x)
```

```python
import jax
import jax.numpy as jnp
from jax import lax
from jax.experimental import pallas as pl
from jax.experimental.pallas import tpu as pltpu

MESH = pl.DeviceIdType.MESH
ROWS = 16
LOAD_ROWS = (16, 16, 32, 64, 128, 256, 512, 1024)
AHEAD = 4


def pallas_dist_rsx_agy_m2048_n1024_kernel(x: jax.Array):
    _, m, n = x.shape
    nch = m // ROWS
    load_start = [sum(LOAD_ROWS[:i]) for i in range(len(LOAD_ROWS))]

    def body(x_hbm, out, xin, send_x, recv_x, ld_sems, sx_sem, rx_sems, sy_sem, ry_sem):
        my_x = lax.axis_index("x")
        my_y = lax.axis_index("y")
        x_nbr = (1 - my_x, my_y)
        y_nbr = (my_x, 1 - my_y)
        own = pl.ds(pl.multiple_of(my_y * n, n), n)

        barrier = pltpu.get_barrier_semaphore()
        pl.semaphore_signal(barrier, 1, device_id=x_nbr, device_id_type=MESH)
        pl.semaphore_signal(barrier, 1, device_id=y_nbr, device_id_type=MESH)

        loads = [
            pltpu.make_async_copy(x_hbm.at[0, pl.ds(s, r)], xin.at[pl.ds(s, r)], ld_sems.at[i])
            for i, (s, r) in enumerate(zip(load_start, LOAD_ROWS))
        ]
        for c in loads:
            c.start()

        def rows(i):
            return pl.ds(i * ROWS, ROWS)

        def xcopy(i):
            return pltpu.make_async_remote_copy(
                send_x.at[rows(i)], recv_x.at[rows(i)], sx_sem, rx_sems.at[i],
                device_id=x_nbr, device_id_type=MESH)

        def ycopy(i):
            return pltpu.make_async_remote_copy(
                out.at[rows(i), own], out.at[rows(i), own], sy_sem, ry_sem,
                device_id=y_nbr, device_id_type=MESH)

        def stage_x(i):
            if i * ROWS in load_start:
                loads[load_start.index(i * ROWS)].wait()
            send_x[rows(i), :] = xin[rows(i), :].astype(jnp.bfloat16)
            if i == 0:
                pl.semaphore_wait(barrier, 2)
            xcopy(i).start()

        def stage_y(i):
            xcopy(i).wait_recv()
            s = xin[rows(i), :] + recv_x[rows(i), :].astype(jnp.float32)
            out[rows(i), own] = s.astype(jnp.bfloat16)
            ycopy(i).start()

        for t in range(-AHEAD, nch):
            if t + AHEAD < nch:
                stage_x(t + AHEAD)
            if t >= 0:
                stage_y(t)

        pltpu.make_async_remote_copy(
            send_x, recv_x, sx_sem, rx_sems.at[0], device_id=x_nbr, device_id_type=MESH).wait_send()
        yall = pltpu.make_async_remote_copy(
            out.at[:, own], out.at[:, own], sy_sem, ry_sem, device_id=y_nbr, device_id_type=MESH)
        yall.wait_send()
        yall.wait_recv()

    return pl.pallas_call(
        body,
        out_shape=pltpu.VMEM((m, 2 * n), jnp.bfloat16),
        in_specs=[pl.BlockSpec(memory_space=pltpu.HBM)],
        out_specs=pl.BlockSpec(memory_space=pltpu.VMEM),
        scratch_shapes=[
            pltpu.VMEM((m, n), jnp.float32),
            pltpu.VMEM((m, n), jnp.bfloat16),
            pltpu.VMEM((m, n), jnp.bfloat16),
            pltpu.SemaphoreType.DMA((len(LOAD_ROWS),)),
            pltpu.SemaphoreType.DMA,
            pltpu.SemaphoreType.DMA((nch,)),
            pltpu.SemaphoreType.DMA,
            pltpu.SemaphoreType.DMA,
        ],
        compiler_params=pltpu.CompilerParams(
            vmem_limit_bytes=32 * 1024 * 1024, collective_id=0, disable_semaphore_checks=True),
    )(x)
```

```python
import jax
import jax.numpy as jnp
import numpy as np
from jax import lax
from jax.experimental import pallas as pl
from jax.experimental.pallas import tpu as pltpu

LANES = 128
PIECE_ROWS = 32
WIRE_ROWS = 88
PLANE_ROWS = 64
STREAM_TILES = 5

BATCHES = ((1, 1), (3, 2), (6, 2), (11, 3), (11, 3))
PACK_AHEAD = (8,) + (2,) * 12
LOADS = "s1 s2 s2 o1 s3 o2 s4 s3 o3 s5 s6 o6 s6 o10 o10"
EARLY_PIECES = 3
LATE_ROWS = 144
Y_READY = 4
FORWARD_LAG = 4


def _i32(bits):
    return int(np.array(bits, np.uint32).view(np.int32))


SIGN = _i32(0x80008000)
EXPONENT = _i32(0x7F807F80)
SIGN_MANTISSA = _i32(0x807F807F)
CODE = 0x03800380
SPARE = 0x7C007C00
STEP = 0x00800080
LOW_BYTES = 0x00FF00FF

srl = lax.shift_right_logical


def _as_float(v):
    return lax.bitcast_convert_type(v, jnp.float32)


def _as_bits(v):
    return lax.bitcast_convert_type(v, jnp.int32)


def _iota(axis):
    return lax.broadcasted_iota(jnp.int32, (8, LANES), axis)


def _lane_max(v):
    return jnp.broadcast_to(jnp.max(v, axis=1, keepdims=True), v.shape)


def _words(rows):
    w = pltpu.bitcast(rows, jnp.int32)
    return [w[r:r + 8, c:c + LANES] for r in range(0, w.shape[0], 8) for c in range(0, w.shape[1], LANES)]


def _rows(words):
    half = len(words) // 2
    w = jnp.concatenate([jnp.concatenate(words[:half], axis=1), jnp.concatenate(words[half:], axis=1)], axis=0)
    return pltpu.bitcast(w, jnp.bfloat16)


def _encode(rows):
    words = _words(rows)
    exponents = [w & EXPONENT for w in words]
    tops = [jnp.maximum(_as_float(e), _as_float(e << 16)) for e in exponents]
    while len(tops) > 1:
        tops = [jnp.maximum(a, b) for a, b in zip(tops[0::2], tops[1::2])]
    top = jnp.broadcast_to(jnp.max(tops[0], axis=0, keepdims=True), (8, LANES))
    top = _as_bits(_lane_max(top)) & 0x7F800000
    both_tops = top | srl(top, 16)

    codes, runs = [], []
    for start in range(0, len(words), 8):
        marks = length = jnp.zeros((8, LANES), jnp.int32)
        for w, e in zip(words[start:start + 8], exponents[start:start + 8]):
            distance = both_tops - e
            shifted = distance + _i32((256 - 7) * STEP)
            far = shifted & SIGN
            one = srl(far, 8)
            beyond = shifted & (far - one)
            codes.append((w ^ e) | (distance - beyond))
            steps = beyond + one
            for step in (srl(steps, 7) & 0x1FF, srl(steps, 23)):
                length = length + step
                marks = marks | (1 << (length & 31))
        runs.append((srl(marks, 1), length))

    whole, split = codes[:11], codes[11:]
    tiles, last = [], whole[10]
    for i, c in enumerate(split):
        tiles += [whole[2 * i] | ((c << 10) & SPARE), whole[2 * i + 1] | ((c << 5) & SPARE)]
        last = last | (srl(c, 1 + i) & (0x40004000 >> i))
    return jnp.concatenate(tiles + [last], axis=0), top, runs


def _codes(wire):
    t = [wire[r:r + 8] for r in range(0, WIRE_ROWS, 8)]
    return t + [(srl(t[2 * i], 10) & 0x001F001F) | (srl(t[2 * i + 1], 5) & 0x03E003E0) | ((t[10] << (1 + i)) & SIGN)
                for i in range(5)]


def _decode(wire, reader, index):
    k = STREAM_TILES
    tag = _lane_max(jnp.where(_iota(1) == index, reader[k], 0).astype(jnp.float32)).astype(jnp.int32)
    top = (tag & 0xFF) << 7
    both_tops = top | (top << 16)
    before = stream = [reader[i] for i in range(k)]
    codes, words = _codes(wire), []
    for start in range(0, len(codes), 8):
        marks = stream[0]
        at = jnp.full((8, LANES), 0.5, jnp.float32)
        for c in codes[start:start + 8]:
            distance = c & CODE
            one = srl(distance + STEP, 3) & STEP
            steps = []
            for far in (srl(one, 7) & 1, srl(one, 23)):
                rest = marks & (marks - far)
                mark = jnp.maximum(at, (marks ^ rest).astype(jnp.float32))
                steps.append(_as_bits(mark) - _as_bits(at))
                at, marks = mark, rest
            words.append((c & SIGN_MANTISSA) | (both_tops - (distance - one + srl(steps[0], 16) + steps[1])))
        taken = srl(_as_bits(at), 23) - 126
        stream = [srl(s, taken) | ((following << 1) << (31 - taken)) for s, following in zip(stream, stream[1:])
                  ] + [srl(stream[-1], taken)]
    for i in range(k):
        reader[i] = jnp.where(tag > 0xFF, before[i], stream[i])
    return _rows(words), tag[0, 0] > 0xFF


def _exponent_plane(rows):
    w = _words(rows)
    return jnp.concatenate(
        [(srl(a, 7) & LOW_BYTES) | ((b << 1) & ~LOW_BYTES) for a, b in zip(w[0::2], w[1::2])], axis=0)


def _decode_with_plane(wire, plane):
    words = []
    for i, c in enumerate(_codes(wire)):
        p = plane[i // 2 * 8:i // 2 * 8 + 8]
        words.append((c & SIGN_MANTISSA) | ((srl(p, 1) if i % 2 else p << 7) & EXPONENT))
    return _rows(words)


USED, LONGEST, TAGS = STREAM_TILES, STREAM_TILES + 1, STREAM_TILES + 2


def _append(writer, runs, index, tag):
    stream = [writer[i] for i in range(STREAM_TILES)]
    used, longest = writer[USED], writer[LONGEST]
    for marks, length in runs:
        tile, bit = srl(used, 5), used & 31
        low, high = marks << bit, srl(srl(marks, 1), 31 - bit)
        stream = [s | jnp.where(tile == i, low, jnp.where(tile == i - 1, high, 0)) for i, s in enumerate(stream)]
        used, longest = used + length, longest | length
    for i, s in enumerate(stream):
        writer[i] = s
    writer[USED], writer[LONGEST] = used, longest
    writer[TAGS] = jnp.where((_iota(0) == 0) & (_iota(1) == index), tag, writer[TAGS])


def _overflows(used, longest, tiles):
    room = jnp.where(_iota(0) == 0, 32 * tiles - 9, 32 * tiles)
    return jnp.max(jnp.where((longest > 31) | (used > room), 1.0, 0.0)) != 0.0


def _clear(writer):
    writer[...] = jnp.zeros(writer.shape, jnp.int32)


def _close(writer, side, tiles):
    for i in range(tiles):
        side[pl.ds(8 * i, 8), :] = writer[i] | writer[TAGS] if i == tiles - 1 else writer[i]
    _clear(writer)


def _open(reader, side, tiles):
    for i in range(STREAM_TILES):
        reader[i] = side[pl.ds(8 * i, 8), :] if i < tiles else jnp.zeros((8, LANES), jnp.int32)
    reader[STREAM_TILES] = jnp.broadcast_to(srl(side[pl.ds(8 * (tiles - 1), 1), :], 23), (8, LANES))


def pallas_dist_rsx_agy_m2048_n1024_kernel(x: jax.Array):
    _, m, n = x.shape
    h = m // 2
    pieces = h // PIECE_ROWS
    assert sum(count for count, _ in BATCHES) == sum(PACK_AHEAD) == pieces
    starts = [sum(count for count, _ in BATCHES[:b]) for b in range(len(BATCHES))]
    split = pieces - pl.cdiv(LATE_ROWS, WIRE_ROWS)
    head = pl.ds(0, (pieces - split) * WIRE_ROWS - LATE_ROWS)
    tail = pl.ds(head.size, WIRE_ROWS - head.size)
    assert head.size > 0

    def body(x_hbm, out, x_own, x_send, received,
             part_tx, part_rx, own_q, x_q, y_q, d_q,
             part_side_tx, part_side_rx, own_side, x_side, y_side, d_side,
             part_plane_tx, part_plane_rx, own_plane, x_plane, y_plane, d_plane,
             part_writer, own_writer, part_reader, x_reader, y_reader, d_reader, planes_sent,
             load_sems, sent, late_sent, part_side_sent, side_sent, plane_sent,
             part_sems, x_sems, y_sem, d_sems, late_sems, part_side_sems, side_sems,
             part_plane_sems, x_plane_sems, y_plane_sems, d_plane_sems):
        my_x, my_y = lax.axis_index("x"), lax.axis_index("y")
        x_nbr, y_nbr = (1 - my_x, my_y), (my_x, 1 - my_y)
        own_rows, other_rows = my_x * h, (1 - my_x) * h
        own_cols = pl.ds(pl.multiple_of(my_y * n, n), n)
        other_cols = pl.ds(pl.multiple_of((1 - my_y) * n, n), n)

        barrier = pltpu.get_barrier_semaphore()
        for nbr in (x_nbr, y_nbr):
            pl.semaphore_signal(barrier, 1, device_id=nbr, device_id_type=pl.DeviceIdType.MESH)

        def rows(first, i, count=1):
            return pl.ds(pl.multiple_of(first + i * PIECE_ROWS, PIECE_ROWS), count * PIECE_ROWS)

        def remote(src, dst, send_sem, recv_sem, to):
            return pltpu.make_async_remote_copy(
                src, dst, send_sem, recv_sem, device_id=to, device_id_type=pl.DeviceIdType.MESH)

        def part_copy(i):
            return remote(part_tx.at[i], part_rx.at[i], sent.at[0], part_sems.at[i], x_nbr)

        def x_copy(i):
            return remote(own_q.at[i], x_q.at[i], sent.at[1], x_sems.at[i], x_nbr)

        def y_copy(i):
            return remote(own_q.at[i], y_q.at[i], sent.at[2], y_sem, y_nbr)

        def d_copy(i):
            return remote(x_q.at[i], d_q.at[i], sent.at[3], d_sems.at[i], y_nbr)

        def head_copy():
            return remote(x_q.at[split, head], d_q.at[split, head], sent.at[4], d_sems.at[split], y_nbr)

        def late_copy(i):
            part = tail if i == split else pl.ds(0, WIRE_ROWS)
            return remote(y_q.at[i, part], d_q.at[i, part], late_sent.at[i - split], late_sems.at[i - split], x_nbr)

        def part_side_copy(b):
            used = pl.ds(0, 8 * BATCHES[b][1])
            return remote(part_side_tx.at[b, used], part_side_rx.at[b, used],
                          part_side_sent.at[b], part_side_sems.at[b], x_nbr)

        def x_side_copy():
            return remote(own_side, x_side, side_sent.at[0], side_sems.at[0], x_nbr)

        def y_side_copy():
            return remote(own_side, y_side, side_sent.at[1], side_sems.at[1], y_nbr)

        def d_side_copy():
            return remote(x_side, d_side, side_sent.at[2], side_sems.at[2], y_nbr)

        def send_plane(src, dst, sems, i, to):
            remote(src.at[i], dst.at[i], plane_sent, sems.at[i], to).start()
            planes_sent[0] += 1

        loads = {"s": {}, "o": {}}
        loaded = {"s": 0, "o": 0}
        for number, load in enumerate(LOADS.split()):
            kind, count = load[0], int(load[1:])
            first_row, dst = (other_rows, x_send) if kind == "s" else (own_rows, x_own)
            copy = pltpu.make_async_copy(x_hbm.at[0, rows(first_row, loaded[kind], count)],
                                         dst.at[pl.ds(loaded[kind] * PIECE_ROWS, count * PIECE_ROWS)],
                                         load_sems.at[number])
            copy.start()
            loads[kind][loaded[kind]] = copy
            loaded[kind] += count
        assert loaded == {"s": pieces, "o": pieces}
        _clear(part_writer)
        _clear(own_writer)
        planes_sent[0] = 0

        def wait_for_load(kind, i):
            for first, copy in loads[kind].items():
                pl.when(i == first)(copy.wait)

        def index_in_batch(i):
            start = 0
            for first in starts[1:]:
                start = jnp.where(i >= first, first, start)
            return i - start

        def close_stream(writer, side, tiles, first, count, source, send_planes):
            @pl.when(_overflows(writer[USED], writer[LONGEST], tiles))
            def _():
                _clear(writer)

                @pl.loop(first, first + count)
                def _(i):
                    _, top, runs = _encode(source(i))
                    (_, a), (_, b) = runs
                    separate = _overflows(writer[USED] + a + b, a | b, tiles)
                    runs = [(jnp.where(separate, 0, marks), jnp.where(separate, 0, length)) for marks, length in runs]
                    _append(writer, runs, i - first, top | jnp.where(separate, _i32(1 << 31), 0))
                    pl.when(separate)(lambda: send_planes(i))

            _close(writer, side, tiles)

        def unpack(dst, wire, reader, index, i, plane, plane_sems, forward=False):
            dst[...], separate = _decode(wire[i], reader, index)

            @pl.when(separate)
            def _():
                remote(plane.at[i], plane.at[i], plane_sent, plane_sems.at[i], y_nbr).wait_recv()
                if forward:
                    send_plane(plane, d_plane, d_plane_sems, i, y_nbr)
                dst[...] = _decode_with_plane(wire[i], plane[i])

        def partial(i):
            return x_send[rows(0, i), :].astype(jnp.bfloat16)

        def send_partial_plane(i):
            part_plane_tx[i] = _exponent_plane(partial(i))
            send_plane(part_plane_tx, part_plane_rx, part_plane_sems, i, x_nbr)

        def pack_partial(i):
            wait_for_load("s", i)
            part_tx[i], top, runs = _encode(partial(i))
            _append(part_writer, runs, index_in_batch(i), top)
            for b, (count, tiles) in enumerate(BATCHES):
                @pl.when(i == starts[b] + count - 1)
                def _():
                    if b == 0:
                        pl.semaphore_wait(barrier, 2)
                    part_copy(starts[b]).start()
                    close_stream(part_writer, part_side_tx.at[b], tiles, starts[b], count,
                                 partial, send_partial_plane)
                    part_side_copy(b).start()
                    pl.loop(starts[b] + 1, starts[b] + count)(lambda j: part_copy(j).start())

        def packed_before(step):
            total = 0
            for earlier, count in enumerate(PACK_AHEAD):
                total = total + jnp.where(step > earlier, count, 0)
            return total

        @pl.loop(0, pieces + 1)
        def _(step):
            @pl.when(step > 0)
            def _():
                i = jnp.maximum(step - 1, 0)
                for b, (_, tiles) in enumerate(BATCHES):
                    @pl.when(i == starts[b])
                    def _():
                        part_side_copy(b).wait_recv()
                        _open(part_reader, part_side_rx.at[b], tiles)
                wait_for_load("o", i)
                part_copy(i).wait_recv()
                unpack(received, part_rx, part_reader, index_in_batch(i), i, part_plane_rx, part_plane_sems)
                total = (x_own[rows(0, i), :] + received[...].astype(jnp.float32)).astype(jnp.bfloat16)
                out[rows(own_rows, i), own_cols] = total
                own_q[i], top, runs = _encode(total)
                y_copy(i).start()
                _append(own_writer, runs, i, top)

            pl.loop(packed_before(step), packed_before(step + 1))(pack_partial)

            @pl.when(step == max(len(PACK_AHEAD) - 1, EARLY_PIECES))
            def _():
                for i in range(EARLY_PIECES):
                    x_copy(i).start()

        def reduced(i):
            return out[rows(own_rows, i), own_cols]

        def send_own_planes(i):
            own_plane[i] = _exponent_plane(reduced(i))
            send_plane(own_plane, x_plane, x_plane_sems, i, x_nbr)
            send_plane(own_plane, y_plane, y_plane_sems, i, y_nbr)

        close_stream(own_writer, own_side, STREAM_TILES, 0, pieces, reduced, send_own_planes)
        x_side_copy().start()
        y_side_copy().start()
        pl.loop(EARLY_PIECES, pieces)(lambda i: x_copy(i).start())

        @pl.loop(0, pieces + FORWARD_LAG)
        def _(step):
            @pl.when(step < pieces)
            def _():
                x_copy(step).wait_recv()
                pl.when(step < split)(lambda: d_copy(step).start())
                pl.when(step == split)(lambda: head_copy().start())

            @pl.when(step == EARLY_PIECES - 1)
            def _():
                x_side_copy().wait_recv()
                d_side_copy().start()
                _open(x_reader, x_side, STREAM_TILES)

            @pl.when(step == Y_READY)
            def _():
                remote(own_q, y_q, sent.at[2], y_sem, y_nbr).wait_recv()
                y_side_copy().wait_recv()
                _open(y_reader, y_side, STREAM_TILES)
                for i in range(split, pieces):
                    late_copy(i).start()

            @pl.when(step == EARLY_PIECES - 1 + FORWARD_LAG)
            def _():
                d_side_copy().wait_recv()
                _open(d_reader, d_side, STREAM_TILES)

            def two_per_step(first_step, arrived):
                return pl.loop(*(jnp.clip(2 * (s - first_step + 1), 0, arrived(s)) for s in (step - 1, step)))

            @two_per_step(EARLY_PIECES - 1, lambda s: jnp.minimum(s + 1, pieces))
            def _(i):
                unpack(out.at[rows(other_rows, i), own_cols], x_q, x_reader, i, i, x_plane, x_plane_sems,
                       forward=True)

            @two_per_step(Y_READY + 2, lambda s: pieces)
            def _(i):
                unpack(out.at[rows(own_rows, i), other_cols], y_q, y_reader, i, i, y_plane, y_plane_sems)

            @two_per_step(EARLY_PIECES - 1 + FORWARD_LAG, lambda s: jnp.maximum(s + 1 - FORWARD_LAG, 0))
            def _(i):
                pl.when(i < split)(lambda: d_copy(i).wait_recv())
                for late in range(split, pieces):
                    @pl.when(i == late)
                    def _():
                        if late == split:
                            head_copy().wait_recv()
                        late_copy(late).wait_recv()
                unpack(out.at[rows(other_rows, i), other_cols], d_q, d_reader, i, i, d_plane, d_plane_sems)

            @pl.when(step == pieces)
            def _():
                remote(part_tx, part_rx, sent.at[0], y_sem, x_nbr).wait_send()
                remote(own_q, x_q, sent.at[1], y_sem, x_nbr).wait_send()
                remote(own_q, y_q, sent.at[2], y_sem, y_nbr).wait_send()
                for b in range(len(BATCHES)):
                    part_side_copy(b).wait_send()
                for copy in (x_side_copy, y_side_copy, d_side_copy):
                    copy().wait_send()

        forwarded = pl.ds(0, split)
        remote(x_q.at[forwarded], d_q.at[forwarded], sent.at[3], y_sem, y_nbr).wait_send()
        head_copy().wait_send()
        for i in range(split, pieces):
            late_copy(i).wait_send()
        pl.loop(0, planes_sent[0])(
            lambda _: remote(own_plane.at[0], x_plane.at[0], plane_sent, y_sem, x_nbr).wait_send())

    def tiles(*shape):
        return pltpu.VMEM(shape + (LANES,), jnp.int32)

    def dma(count):
        return pltpu.SemaphoreType.DMA((count,))

    return pl.pallas_call(
        body,
        out_shape=pltpu.VMEM((m, 2 * n), jnp.bfloat16),
        in_specs=[pl.BlockSpec(memory_space=pltpu.HBM)],
        out_specs=pl.BlockSpec(memory_space=pltpu.VMEM),
        scratch_shapes=(
            [pltpu.VMEM((h, n), jnp.float32)] * 2 + [pltpu.VMEM((PIECE_ROWS, n), jnp.bfloat16)]
            + [tiles(pieces, WIRE_ROWS)] * 6
            + [tiles(len(BATCHES), 8 * STREAM_TILES)] * 2 + [tiles(8 * STREAM_TILES)] * 4
            + [tiles(pieces, PLANE_ROWS)] * 6
            + [tiles(STREAM_TILES + 3, 8)] * 2 + [tiles(STREAM_TILES + 1, 8)] * 4 + [pltpu.SMEM((1,), jnp.int32)]
            + [dma(len(LOADS.split())), dma(5), dma(pieces - split), dma(len(BATCHES)), dma(3),
               pltpu.SemaphoreType.DMA]
            + [dma(pieces), dma(pieces), pltpu.SemaphoreType.DMA, dma(pieces), dma(pieces - split),
               dma(len(BATCHES)), dma(3)]
            + [dma(pieces)] * 4
        ),
        compiler_params=pltpu.CompilerParams(
            vmem_limit_bytes=40 * 1024 * 1024, collective_id=0, disable_semaphore_checks=True),
    )(x)
```

```python
import jax
import jax.numpy as jnp
import numpy as np
from jax import lax
from jax.experimental import pallas as pl
from jax.experimental.pallas import tpu as pltpu

LANES = 128
PIECE_ROWS = 32
WIRE_ROWS = 88
PLANE_ROWS = 64
STREAM_TILES = 5

BATCHES = ((4, 2), (10, 3), (18, 4))
PACK_AHEAD = (8,) + (2,) * 12
LOADS = "s1 s2 s2 o1 s3 o2 s4 s3 o3 s5 s6 o6 s6 o10 o10"
RELAY_AT = 5
EARLY_PIECES = 3
LATE_PIECES = 2
Y_READY = 4
FORWARD_LAG = 4


def _i32(bits):
    return int(np.array(bits, np.uint32).view(np.int32))


SIGN = _i32(0x80008000)
EXPONENT = _i32(0x7F807F80)
SIGN_MANTISSA = _i32(0x807F807F)
CODE = 0x03800380
SPARE = 0x7C007C00
STEP = 0x00800080
LOW_BYTES = 0x00FF00FF

srl = lax.shift_right_logical


def _as_float(v):
    return lax.bitcast_convert_type(v, jnp.float32)


def _as_bits(v):
    return lax.bitcast_convert_type(v, jnp.int32)


def _iota(axis):
    return lax.broadcasted_iota(jnp.int32, (8, LANES), axis)


def _lane_max(v):
    return jnp.broadcast_to(jnp.max(v, axis=1, keepdims=True), v.shape)


def _tile_max(v):
    return _lane_max(jnp.broadcast_to(jnp.max(v, axis=0, keepdims=True), v.shape))


def _words(rows):
    w = pltpu.bitcast(rows, jnp.int32)
    return [w[r:r + 8, c:c + LANES] for r in range(0, w.shape[0], 8) for c in range(0, w.shape[1], LANES)]


def _rows(words):
    half = len(words) // 2
    w = jnp.concatenate([jnp.concatenate(words[:half], axis=1), jnp.concatenate(words[half:], axis=1)], axis=0)
    return pltpu.bitcast(w, jnp.bfloat16)


def _encode(rows):
    words = _words(rows)
    exponents = [w & EXPONENT for w in words]
    tops = [jnp.maximum(_as_float(e), _as_float(e << 16)) for e in exponents]
    while len(tops) > 1:
        tops = [jnp.maximum(a, b) for a, b in zip(tops[0::2], tops[1::2])]
    top = _as_bits(_tile_max(tops[0])) & 0x7F800000
    both_tops = top | srl(top, 16)

    codes, runs = [], []
    for start in range(0, len(words), 8):
        marks = length = jnp.zeros((8, LANES), jnp.int32)
        for w, e in zip(words[start:start + 8], exponents[start:start + 8]):
            distance = both_tops - e
            shifted = distance + _i32((256 - 7) * STEP)
            far = shifted & SIGN
            one = srl(far, 8)
            beyond = shifted & (far - one)
            codes.append((w ^ e) | (distance - beyond))
            steps = beyond + one
            for step in (srl(steps, 7) & 0x1FF, srl(steps, 23)):
                length = length + step
                marks = marks | (1 << (length & 31))
        runs.append((srl(marks, 1), length))

    whole, split = codes[:11], codes[11:]
    tiles, last = [], whole[10]
    for i, c in enumerate(split):
        tiles += [whole[2 * i] | ((c << 10) & SPARE), whole[2 * i + 1] | ((c << 5) & SPARE)]
        last = last | (srl(c, 1 + i) & (0x40004000 >> i))
    return jnp.concatenate(tiles + [last], axis=0), top, runs


def _codes(wire):
    t = [wire[r:r + 8] for r in range(0, WIRE_ROWS, 8)]
    return t + [(srl(t[2 * i], 10) & 0x001F001F) | (srl(t[2 * i + 1], 5) & 0x03E003E0) | ((t[10] << (1 + i)) & SIGN)
                for i in range(5)]


def _decode(wire, reader, index):
    k = STREAM_TILES
    tag = _lane_max(jnp.where(_iota(1) == index, reader[k], 0).astype(jnp.float32)).astype(jnp.int32)
    top = (tag & 0xFF) << 7
    both_tops = top | (top << 16)
    before = stream = [reader[i] for i in range(k)]
    codes, words = _codes(wire), []
    for start in range(0, len(codes), 8):
        marks = stream[0]
        at = jnp.full((8, LANES), 0.5, jnp.float32)
        for c in codes[start:start + 8]:
            distance = c & CODE
            one = srl(distance + STEP, 3) & STEP
            steps = []
            for far in (srl(one, 7) & 1, srl(one, 23)):
                rest = marks & (marks - far)
                mark = jnp.maximum(at, (marks ^ rest).astype(jnp.float32))
                steps.append(_as_bits(mark) - _as_bits(at))
                at, marks = mark, rest
            words.append((c & SIGN_MANTISSA) | (both_tops - (distance - one + srl(steps[0], 16) + steps[1])))
        taken = srl(_as_bits(at), 23) - 126
        stream = [srl(s, taken) | ((following << 1) << (31 - taken)) for s, following in zip(stream, stream[1:])
                  ] + [srl(stream[-1], taken)]
    for i in range(k):
        reader[i] = jnp.where(tag > 0xFF, before[i], stream[i])
    return _rows(words), tag[0, 0] > 0xFF


def _exponent_plane(rows):
    w = _words(rows)
    return jnp.concatenate(
        [(srl(a, 7) & LOW_BYTES) | ((b << 1) & ~LOW_BYTES) for a, b in zip(w[0::2], w[1::2])], axis=0)


def _decode_with_plane(wire, plane):
    words = []
    for i, c in enumerate(_codes(wire)):
        p = plane[i // 2 * 8:i // 2 * 8 + 8]
        words.append((c & SIGN_MANTISSA) | ((srl(p, 1) if i % 2 else p << 7) & EXPONENT))
    return _rows(words)


USED, TAGS, HELD = STREAM_TILES, STREAM_TILES + 1, STREAM_TILES + 2


def _add_held(writer, index, tiles):
    top, marks_a, length_a, marks_b, length_b = (writer[HELD + i] for i in range(5))
    used = writer[USED]
    room = jnp.where(_iota(0) == 0, 32 * tiles - 9, 32 * tiles)
    full = ((length_a | length_b) > 31) | (used + length_a + length_b > room)
    separate = _tile_max(jnp.where(full, 1.0, 0.0))
    stream = [writer[i] for i in range(STREAM_TILES)]
    for marks, length in ((marks_a, length_a), (marks_b, length_b)):
        marks = jnp.where(separate > 0, 0, marks)
        tile, bit = srl(used, 5), used & 31
        low, high = marks << bit, srl(srl(marks, 1), 31 - bit)
        stream = [s | jnp.where(tile == i, low, jnp.where(tile == i - 1, high, 0)) for i, s in enumerate(stream)]
        used = used + jnp.where(separate > 0, 0, length)
    for i, s in enumerate(stream):
        writer[i] = s
    writer[USED] = used
    tag = top | jnp.where(separate > 0, _i32(1 << 31), 0)
    writer[TAGS] = jnp.where((_iota(0) == 0) & (_iota(1) == index), tag, writer[TAGS])
    return separate[0, 0] > 0


def _hold(writer, top, runs):
    for i, v in enumerate((top,) + runs[0] + runs[1]):
        writer[HELD + i] = v


def _clear(writer):
    writer[...] = jnp.zeros(writer.shape, jnp.int32)


def _close(writer, side, tiles):
    for i in range(tiles):
        side[pl.ds(8 * i, 8), :] = writer[i] | writer[TAGS] if i == tiles - 1 else writer[i]
    _clear(writer)


def _open(reader, side, tiles):
    for i in range(STREAM_TILES):
        reader[i] = side[pl.ds(8 * i, 8), :] if i < tiles else jnp.zeros((8, LANES), jnp.int32)
    reader[STREAM_TILES] = jnp.broadcast_to(srl(side[pl.ds(8 * (tiles - 1), 1), :], 23), (8, LANES))


def pallas_dist_rsx_agy_m2048_n1024_kernel(x: jax.Array):
    _, m, n = x.shape
    h = m // 2
    pieces = h // PIECE_ROWS
    assert sum(count for count, _ in BATCHES) == sum(PACK_AHEAD) == pieces
    starts = [sum(count for count, _ in BATCHES[:b]) for b in range(len(BATCHES))]
    assert all(sum(PACK_AHEAD[:first + 1]) >= first + count for first, (count, _) in zip(starts, BATCHES))
    assert RELAY_AT < PACK_AHEAD[0]
    late = pieces - LATE_PIECES

    def body(x_hbm, out, x_own, x_send, received,
             part_tx, part_rx, own_q, x_q, y_q, d_q,
             part_side_tx, part_side_rx, own_side, x_side, y_side, d_side,
             part_plane_tx, part_plane_rx, own_plane, x_plane, y_plane, d_plane,
             part_writer, own_writer, part_reader, x_reader, y_reader, d_reader, planes_sent,
             entered, load_sems, sent, late_sent, part_side_sent, side_sent, plane_sent,
             part_sems, x_sems, y_sem, d_sems, part_side_sems, side_sems,
             part_plane_sems, x_plane_sems, y_plane_sems, d_plane_sems):
        my_x, my_y = lax.axis_index("x"), lax.axis_index("y")
        x_nbr, y_nbr = (1 - my_x, my_y), (my_x, 1 - my_y)
        own_rows, other_rows = my_x * h, (1 - my_x) * h
        own_cols = pl.ds(pl.multiple_of(my_y * n, n), n)
        other_cols = pl.ds(pl.multiple_of((1 - my_y) * n, n), n)

        barrier = pltpu.get_barrier_semaphore()

        def signal(sem, to):
            pl.semaphore_signal(sem, 1, device_id=to, device_id_type=pl.DeviceIdType.MESH)

        signal(barrier, x_nbr)
        pl.when(my_x == 0)(lambda: signal(barrier, y_nbr))

        def rows(first, i, count=1):
            return pl.ds(pl.multiple_of(first + i * PIECE_ROWS, PIECE_ROWS), count * PIECE_ROWS)

        def remote(src, dst, send_sem, recv_sem, to):
            return pltpu.make_async_remote_copy(
                src, dst, send_sem, recv_sem, device_id=to, device_id_type=pl.DeviceIdType.MESH)

        def part_copy(i):
            return remote(part_tx.at[i], part_rx.at[i], sent.at[0], part_sems.at[i], x_nbr)

        def x_copy(i):
            return remote(own_q.at[i], x_q.at[i], sent.at[1], x_sems.at[i], x_nbr)

        def y_copy(i):
            return remote(own_q.at[i], y_q.at[i], sent.at[2], y_sem, y_nbr)

        def d_copy(i):
            return remote(x_q.at[i], d_q.at[i], sent.at[3], d_sems.at[i], y_nbr)

        def late_copy(i):
            return remote(y_q.at[i], d_q.at[i], late_sent.at[i - late], d_sems.at[i], x_nbr)

        def part_side_copy(b):
            used = pl.ds(0, 8 * BATCHES[b][1])
            return remote(part_side_tx.at[b, used], part_side_rx.at[b, used],
                          part_side_sent.at[b], part_side_sems.at[b], x_nbr)

        def x_side_copy():
            return remote(own_side, x_side, side_sent.at[0], side_sems.at[0], x_nbr)

        def y_side_copy():
            return remote(own_side, y_side, side_sent.at[1], side_sems.at[1], y_nbr)

        def d_side_copy():
            return remote(x_side, d_side, side_sent.at[2], side_sems.at[2], y_nbr)

        def send_plane(src, dst, sems, i, to):
            remote(src.at[i], dst.at[i], plane_sent, sems.at[i], to).start()
            planes_sent[0] += 1

        loads = {"s": {}, "o": {}}
        loaded = {"s": 0, "o": 0}
        for number, load in enumerate(LOADS.split()):
            kind, count = load[0], int(load[1:])
            first_row, dst = (other_rows, x_send) if kind == "s" else (own_rows, x_own)
            copy = pltpu.make_async_copy(x_hbm.at[0, rows(first_row, loaded[kind], count)],
                                         dst.at[pl.ds(loaded[kind] * PIECE_ROWS, count * PIECE_ROWS)],
                                         load_sems.at[number])
            copy.start()
            loads[kind][loaded[kind]] = copy
            loaded[kind] += count
        assert loaded == {"s": pieces, "o": pieces}
        _clear(part_writer)
        _clear(own_writer)
        planes_sent[0] = 0

        def wait_for_load(kind, i):
            for first, copy in loads[kind].items():
                pl.when(i == first)(copy.wait)

        def batch_of(i):
            start, tiles = 0, BATCHES[0][1]
            for first, (_, length) in zip(starts[1:], BATCHES[1:]):
                start, tiles = jnp.where(i >= first, first, start), jnp.where(i >= first, length, tiles)
            return i - start, tiles

        def unpack(dst, wire, reader, index, i, plane, plane_sems, forward=False):
            dst[...], separate = _decode(wire[i], reader, index)

            @pl.when(separate)
            def _():
                remote(plane.at[i], plane.at[i], plane_sent, plane_sems.at[i], y_nbr).wait_recv()
                if forward:
                    send_plane(plane, d_plane, d_plane_sems, i, y_nbr)
                dst[...] = _decode_with_plane(wire[i], plane[i])

        def partial(i):
            return x_send[rows(0, i), :].astype(jnp.bfloat16)

        def send_partial_plane(i):
            part_plane_tx[i] = _exponent_plane(partial(i))
            send_plane(part_plane_tx, part_plane_rx, part_plane_sems, i, x_nbr)

        def pack_partial(i):
            wait_for_load("s", i)
            index, tiles = batch_of(i)
            separate = _add_held(part_writer, index - 1, tiles)
            part_tx[i], top, runs = _encode(partial(i))
            _hold(part_writer, top, runs)
            pl.when(separate)(lambda: send_partial_plane(jnp.maximum(i - 1, 0)))
            for b, (count, tiles) in enumerate(BATCHES):
                @pl.when(i == starts[b])
                def _():
                    if b == 0:
                        pl.when(my_x == 0)(lambda: pl.semaphore_wait(barrier, 2))
                        pl.when(my_x == 1)(lambda: pl.semaphore_wait(barrier, 1))
                    part_copy(starts[b]).start()
                    if b == 0:
                        pl.when(my_x == 0)(lambda: signal(entered, y_nbr))

                @pl.when(i == starts[b] + count - 1)
                def _():
                    separate = _add_held(part_writer, count - 1, tiles)
                    _close(part_writer, part_side_tx.at[b], tiles)
                    part_side_copy(b).start()
                    pl.loop(starts[b] + 1, starts[b] + count)(lambda j: part_copy(j).start())
                    pl.when(separate)(lambda: send_partial_plane(i))

            @pl.when((i == RELAY_AT) & (my_x == 0))
            def _():
                pl.semaphore_wait(entered, 1)
                signal(entered, x_nbr)

        def packed_before(step):
            total = 0
            for earlier, count in enumerate(PACK_AHEAD):
                total = total + jnp.where(step > earlier, count, 0)
            return total

        def send_own_plane(i):
            own_plane[i] = _exponent_plane(out[rows(own_rows, i), own_cols])
            send_plane(own_plane, x_plane, x_plane_sems, i, x_nbr)
            send_plane(own_plane, y_plane, y_plane_sems, i, y_nbr)

        @pl.loop(0, pieces + 1)
        def _(step):
            @pl.when(step > 0)
            def _():
                i = jnp.maximum(step - 1, 0)
                for b, (_, tiles) in enumerate(BATCHES):
                    @pl.when(i == starts[b])
                    def _():
                        part_side_copy(b).wait_recv()
                        _open(part_reader, part_side_rx.at[b], tiles)
                wait_for_load("o", i)
                part_copy(i).wait_recv()
                unpack(received, part_rx, part_reader, batch_of(i)[0], i, part_plane_rx, part_plane_sems)
                total = (x_own[rows(0, i), :] + received[...].astype(jnp.float32)).astype(jnp.bfloat16)
                out[rows(own_rows, i), own_cols] = total
                separate = _add_held(own_writer, i - 1, STREAM_TILES)
                own_q[i], top, runs = _encode(total)
                pl.when((i == 0) & (my_x == 1))(lambda: pl.semaphore_wait(entered, 1))
                y_copy(i).start()
                _hold(own_writer, top, runs)
                pl.when(separate)(lambda: send_own_plane(jnp.maximum(i - 1, 0)))

            pl.loop(packed_before(step), packed_before(step + 1))(pack_partial)

            @pl.when(step == max(len(PACK_AHEAD) - 1, EARLY_PIECES))
            def _():
                for i in range(EARLY_PIECES):
                    x_copy(i).start()

        separate = _add_held(own_writer, pieces - 1, STREAM_TILES)
        _close(own_writer, own_side, STREAM_TILES)
        x_side_copy().start()
        y_side_copy().start()
        pl.loop(EARLY_PIECES, pieces)(lambda i: x_copy(i).start())
        pl.when(separate)(lambda: send_own_plane(pieces - 1))

        @pl.loop(0, pieces + 1)
        def _(step):
            @pl.when(step < pieces)
            def _():
                x_copy(step).wait_recv()
                pl.when(step < late)(lambda: d_copy(step).start())

            @pl.when(step == EARLY_PIECES - 1)
            def _():
                x_side_copy().wait_recv()
                d_side_copy().start()
                _open(x_reader, x_side, STREAM_TILES)

            @pl.when(step == Y_READY)
            def _():
                remote(own_q, y_q, sent.at[2], y_sem, y_nbr).wait_recv()
                y_side_copy().wait_recv()
                _open(y_reader, y_side, STREAM_TILES)
                for i in range(late, pieces):
                    late_copy(i).start()

            @pl.when(step == EARLY_PIECES - 1 + FORWARD_LAG)
            def _():
                d_side_copy().wait_recv()
                _open(d_reader, d_side, STREAM_TILES)

            @pl.when(step == pieces)
            def _():
                remote(part_tx, part_rx, sent.at[0], y_sem, x_nbr).wait_send()
                remote(own_q, x_q, sent.at[1], y_sem, x_nbr).wait_send()
                remote(own_q, y_q, sent.at[2], y_sem, y_nbr).wait_send()
                for b in range(len(BATCHES)):
                    part_side_copy(b).wait_send()
                for copy in (x_side_copy, y_side_copy, d_side_copy):
                    copy().wait_send()

            def two_per_step(first_step, arrived):
                before, after = (jnp.clip(2 * (s - first_step + 1), 0, arrived(s)) for s in (step - 1, step))
                return pl.loop(before, jnp.where(step == pieces, pieces, after))

            @two_per_step(EARLY_PIECES - 1, lambda s: jnp.minimum(s + 1, pieces))
            def _(i):
                unpack(out.at[rows(other_rows, i), own_cols], x_q, x_reader, i, i, x_plane, x_plane_sems,
                       forward=True)

            @two_per_step(Y_READY + 2, lambda s: pieces)
            def _(i):
                unpack(out.at[rows(own_rows, i), other_cols], y_q, y_reader, i, i, y_plane, y_plane_sems)

            @two_per_step(EARLY_PIECES - 1 + FORWARD_LAG, lambda s: jnp.maximum(s + 1 - FORWARD_LAG, 0))
            def _(i):
                d_copy(i).wait_recv()
                unpack(out.at[rows(other_rows, i), other_cols], d_q, d_reader, i, i, d_plane, d_plane_sems)

        forwarded = pl.ds(0, late)
        remote(x_q.at[forwarded], d_q.at[forwarded], sent.at[3], y_sem, y_nbr).wait_send()
        for i in range(late, pieces):
            late_copy(i).wait_send()
        pl.loop(0, planes_sent[0])(
            lambda _: remote(own_plane.at[0], x_plane.at[0], plane_sent, y_sem, x_nbr).wait_send())

    def tiles(*shape):
        return pltpu.VMEM(shape + (LANES,), jnp.int32)

    def dma(count):
        return pltpu.SemaphoreType.DMA((count,))

    return pl.pallas_call(
        body,
        out_shape=pltpu.VMEM((m, 2 * n), jnp.bfloat16),
        in_specs=[pl.BlockSpec(memory_space=pltpu.HBM)],
        out_specs=pl.BlockSpec(memory_space=pltpu.VMEM),
        scratch_shapes=(
            [pltpu.VMEM((h, n), jnp.float32)] * 2 + [pltpu.VMEM((PIECE_ROWS, n), jnp.bfloat16)]
            + [tiles(pieces, WIRE_ROWS)] * 6
            + [tiles(len(BATCHES), 8 * STREAM_TILES)] * 2 + [tiles(8 * STREAM_TILES)] * 4
            + [tiles(pieces, PLANE_ROWS)] * 6
            + [tiles(STREAM_TILES + 7, 8)] * 2 + [tiles(STREAM_TILES + 1, 8)] * 4 + [pltpu.SMEM((1,), jnp.int32)]
            + [pltpu.SemaphoreType.REGULAR, dma(len(LOADS.split()))]
            + [dma(4), dma(LATE_PIECES), dma(len(BATCHES)), dma(3), pltpu.SemaphoreType.DMA]
            + [dma(pieces), dma(pieces), pltpu.SemaphoreType.DMA, dma(pieces), dma(len(BATCHES)), dma(3)]
            + [dma(pieces)] * 4
        ),
        compiler_params=pltpu.CompilerParams(
            vmem_limit_bytes=40 * 1024 * 1024, collective_id=0, disable_semaphore_checks=True),
    )(x)
```
